```python
import numpy as np

kernel_name = "dist_argmax_global_i_m4096_n1024"

def setup_inputs():
    return {"x": np.random.randn(16384, 1024).astype(np.float32)}

def reference(x: np.ndarray) -> np.ndarray:
    idx = np.argmax(x, axis=0).astype(np.float32)
    val = np.max(x, axis=0)
    return np.stack([val, idx], axis=0)
```

```python
import jax
import jax.numpy as jnp
from jax import lax
from jax.experimental import pallas as pl
from jax.experimental.pallas import tpu as pltpu

N_DEV = 4
SUB = 8


def pallas_dist_argmax_global_i_m4096_n1024_kernel(
    x: jax.Array,
):
    m, n = x.shape
    tm = 512
    steps = m // tm
    groups = tm // SUB

    def body(x_ref, out_ref, acc_val, acc_grp, comm, send_sems, recv_sems):
        step = pl.program_id(0)
        my = lax.axis_index("i")

        @pl.when(step == 0)
        def _():
            barrier = pltpu.get_barrier_semaphore()
            for d in range(1, N_DEV):
                pl.semaphore_signal(
                    barrier, inc=1, device_id=((my + d) % N_DEV,),
                    device_id_type=pl.DeviceIdType.MESH)
            acc_val[...] = jnp.full((SUB, n), -jnp.inf, jnp.float32)
            acc_grp[...] = jnp.zeros((SUB, n), jnp.int32)

        def grp_body(g, carry):
            val, grp = carry
            xs = x_ref[pl.ds(pl.multiple_of(g * SUB, SUB), SUB), :]
            take = xs > val
            val = jnp.where(take, xs, val)
            grp = jnp.where(take, step * groups + g, grp)
            return val, grp

        val, grp = lax.fori_loop(0, groups, grp_body, (acc_val[...], acc_grp[...]),
                                 unroll=4)
        acc_val[...] = val
        acc_grp[...] = grp

        @pl.when(step == steps - 1)
        def _():
            row = grp * SUB + lax.broadcasted_iota(jnp.int32, (SUB, n), 0)
            best = jnp.max(val, axis=0, keepdims=True)
            cand = jnp.where(val == best, row, m)
            idx = jnp.min(cand, axis=0, keepdims=True) + my * m
            comm[my, 0:1, :] = best
            comm[my, 1:2, :] = idx.astype(jnp.float32)

            barrier = pltpu.get_barrier_semaphore()
            pl.semaphore_wait(barrier, N_DEV - 1)

            sends = []
            for d in range(1, N_DEV):
                peer = (my + d) % N_DEV
                cp = pltpu.make_async_remote_copy(
                    src_ref=comm.at[my], dst_ref=comm.at[my],
                    send_sem=send_sems.at[d - 1], recv_sem=recv_sems.at[my],
                    device_id=(peer,), device_id_type=pl.DeviceIdType.MESH)
                cp.start()
                sends.append(cp)
            for d in range(1, N_DEV):
                peer = (my + d) % N_DEV
                pltpu.make_async_remote_copy(
                    src_ref=comm.at[peer], dst_ref=comm.at[peer],
                    send_sem=send_sems.at[d - 1], recv_sem=recv_sems.at[peer],
                    device_id=(peer,), device_id_type=pl.DeviceIdType.MESH).wait_recv()
            for cp in sends:
                cp.wait_send()

            bv = comm[0, 0:1, :]
            bi = comm[0, 1:2, :]
            for k in range(1, N_DEV):
                v = comm[k, 0:1, :]
                i = comm[k, 1:2, :]
                take = v > bv
                bv = jnp.where(take, v, bv)
                bi = jnp.where(take, i, bi)
            out_ref[0:1, :] = bv
            out_ref[1:2, :] = bi

    return pl.pallas_call(
        body,
        out_shape=jax.ShapeDtypeStruct((2, n), jnp.float32),
        grid=(steps,),
        in_specs=[pl.BlockSpec((tm, n), lambda s: (s, 0))],
        out_specs=pl.BlockSpec((2, n), lambda s: (0, 0)),
        scratch_shapes=[
            pltpu.VMEM((SUB, n), jnp.float32),
            pltpu.VMEM((SUB, n), jnp.int32),
            pltpu.VMEM((N_DEV, 2, n), jnp.float32),
            pltpu.SemaphoreType.DMA((N_DEV - 1,)),
            pltpu.SemaphoreType.DMA((N_DEV,)),
        ],
        compiler_params=pltpu.CompilerParams(
            collective_id=0, dimension_semantics=("arbitrary",)),
    )(x)
```

```python
import jax
import jax.numpy as jnp
from jax import lax
from jax.experimental import pallas as pl
from jax.experimental.pallas import tpu as pltpu

N_DEV = 4
SUB = 8


def _better(new, old):
    return jnp.logical_or(new > old, jnp.logical_and(new != new, old == old))


def pallas_dist_argmax_global_i_m4096_n1024_kernel(
    x: jax.Array,
):
    m, n = x.shape
    tm = 128
    nbuf = 8
    steps = m // tm
    groups = tm // SUB

    def body(x_hbm, out_ref, buf, dsem, comm, send_sems, recv_sems):
        my = lax.axis_index("i")

        barrier = pltpu.get_barrier_semaphore()
        for d in range(1, N_DEV):
            pl.semaphore_signal(barrier, inc=1, device_id=((my + d) % N_DEV,),
                                device_id_type=pl.DeviceIdType.MESH)

        def load(s):
            return pltpu.make_async_copy(
                x_hbm.at[pl.ds(s * tm, tm), :], buf.at[s % nbuf], dsem.at[s % nbuf])

        for s in range(min(nbuf, steps)):
            load(s).start()

        val = jnp.full((SUB, n), -jnp.inf, jnp.float32)
        grp = jnp.zeros((SUB, n), jnp.int32)
        for s in range(steps):
            load(s).wait()
            blk = buf.at[s % nbuf]

            def grp_body(g, carry, blk=blk, s=s):
                val, grp = carry
                xs = blk[pl.ds(pl.multiple_of(g * SUB, SUB), SUB), :]
                take = _better(xs, val)
                return jnp.where(take, xs, val), jnp.where(take, s * groups + g, grp)

            val, grp = lax.fori_loop(0, groups, grp_body, (val, grp), unroll=4)
            if s + nbuf < steps:
                load(s + nbuf).start()

        row = grp * SUB + lax.broadcasted_iota(jnp.int32, (SUB, n), 0)
        isnan = val != val
        nan_cnt = jnp.max(isnan.astype(jnp.int32), axis=0, keepdims=True)
        finite_best = jnp.max(jnp.where(isnan, -jnp.inf, val), axis=0, keepdims=True)
        any_nan8 = jnp.broadcast_to(nan_cnt, (SUB, n)) > 0
        match = jnp.logical_or(
            isnan, jnp.logical_and(jnp.logical_not(any_nan8), val == finite_best))
        idx = jnp.min(jnp.where(match, row, m), axis=0, keepdims=True) + my * m
        comm[my, 0:1, :] = jnp.where(nan_cnt > 0, jnp.nan, finite_best)
        comm[my, 1:2, :] = idx.astype(jnp.float32)

        pl.semaphore_wait(barrier, N_DEV - 1)

        sends = []
        for d in (2, 1, 3):
            peer = (my + d) % N_DEV
            cp = pltpu.make_async_remote_copy(
                src_ref=comm.at[my], dst_ref=comm.at[my],
                send_sem=send_sems.at[d - 1], recv_sem=recv_sems.at[my],
                device_id=(peer,), device_id_type=pl.DeviceIdType.MESH)
            cp.start()
            sends.append(cp)
        for d in range(1, N_DEV):
            peer = (my + d) % N_DEV
            pltpu.make_async_remote_copy(
                src_ref=comm.at[peer], dst_ref=comm.at[peer],
                send_sem=send_sems.at[d - 1], recv_sem=recv_sems.at[peer],
                device_id=(peer,), device_id_type=pl.DeviceIdType.MESH).wait_recv()
        for cp in sends:
            cp.wait_send()

        bv = comm[0, 0:1, :]
        bi = comm[0, 1:2, :]
        for k in range(1, N_DEV):
            v = comm[k, 0:1, :]
            i = comm[k, 1:2, :]
            take = _better(v, bv)
            bv = jnp.where(take, v, bv)
            bi = jnp.where(take, i, bi)
        out_ref[0:1, :] = bv
        out_ref[1:2, :] = bi

    return pl.pallas_call(
        body,
        out_shape=jax.ShapeDtypeStruct((2, n), jnp.float32),
        in_specs=[pl.BlockSpec(memory_space=pl.ANY)],
        out_specs=pl.BlockSpec(memory_space=pltpu.VMEM),
        scratch_shapes=[
            pltpu.VMEM((nbuf, tm, n), jnp.float32),
            pltpu.SemaphoreType.DMA((nbuf,)),
            pltpu.VMEM((N_DEV, 2, n), jnp.float32),
            pltpu.SemaphoreType.DMA((N_DEV - 1,)),
            pltpu.SemaphoreType.DMA((N_DEV,)),
        ],
        compiler_params=pltpu.CompilerParams(collective_id=0),
    )(x)
```
